```python
import numpy as np

kernel_name = "dist_sparse_attn_blocksparse_htp_b2_sq128_skv128_hq4_dh64"

def setup_inputs():
    x = np.random.randn(2, 128, 512).astype(np.float32)
    Wq = np.random.randn(512, 1024).astype(np.float32) * 0.02
    K_ext = np.random.randn(2, 128, 16, 64).astype(np.float32)
    V_ext = np.random.randn(2, 128, 16, 64).astype(np.float32)
    Wo = np.random.randn(1024, 512).astype(np.float32) * 0.02
    return {"x": x, "Wq": Wq, "K_ext": K_ext, "V_ext": V_ext, "Wo": Wo}

def reference(x, Wq, K_ext, V_ext, Wo):
    B, Sq, Skv, Hq, Dh = 2, 128, 128, 16, 64
    Q = (x @ Wq).reshape(B, Sq, Hq, Dh)
    qb = (np.arange(Sq) // 64)[:, None]
    kb = (np.arange(Skv) // 64)[None, :]
    mask = (qb == kb) | (kb == 0) | ((qb + kb) % 3 == 0)
    scores = np.einsum('bihd,bjhd->bhij', Q, K_ext).astype(np.float32) * 0.125
    scores = np.where(mask[None, None, :, :], scores, -1e9)
    scores_max = scores.max(axis=-1, keepdims=True)
    w = np.exp(scores - scores_max)
    row_keep = mask.any(axis=1)
    w_sum = np.where(row_keep[None, None, :, None], w.sum(axis=-1, keepdims=True), 1.0)
    w = w / w_sum
    w = np.where(row_keep[None, None, :, None], w, 0.0)
    ctx = np.einsum('bhij,bjhd->bihd', w, V_ext).reshape(B, Sq, Hq * Dh)
    return ctx @ Wo
```

```python
import jax
import jax.numpy as jnp
from jax import lax
from jax.experimental import pallas as pl
from jax.experimental.pallas import tpu as pltpu

B, SQ, SKV, DM = 2, 128, 128, 512
HL, DH = 4, 64
RB = 64
NR = B * SQ // RB
QC = DM // 4
BF = jnp.bfloat16
F32 = jnp.float32
MESH = pl.DeviceIdType.MESH


def _body(x_hbm, wq_hbm, kt_hbm, vt_hbm, wo_hbm, o_ref,
          x_v, wq_v, kt_v, vt_v, wo_v, wq_b, wo_b, keep,
          sbuf, rbuf, lsem, ssem, rsem):
    me = lax.axis_index("i")
    pa = me ^ 1
    pb = 3 - me
    a = (me ^ (me >> 1)) & 1
    b = me >> 1
    peers = (pa, pb)
    quarters = (1 - a, 3 - b, a, 2 + b)
    cols = [pl.multiple_of(q * QC, QC) for q in quarters]

    bsem = pltpu.get_barrier_semaphore()
    for p in peers:
        pl.semaphore_signal(bsem, inc=1, device_id=(p,), device_id_type=MESH)

    def cx(r):
        return pltpu.make_async_copy(x_hbm.at[r // 2, pl.ds((r % 2) * RB, RB)], x_v.at[r], lsem.at[r])
    def cwq(p):
        return pltpu.make_async_copy(wq_hbm.at[:, pl.ds(p * 128, 128)], wq_v.at[p], lsem.at[4 + p])
    def ck(bb):
        return pltpu.make_async_copy(kt_hbm.at[bb, pl.ds(me * HL, HL)], kt_v.at[bb], lsem.at[6 + bb])
    def cv(bb):
        return pltpu.make_async_copy(vt_hbm.at[bb, pl.ds(me * HL, HL)], vt_v.at[bb], lsem.at[8 + bb])
    def cwo(j):
        return pltpu.make_async_copy(wo_hbm.at[:, pl.ds(cols[j], QC)], wo_v.at[j], lsem.at[10 + j])

    order = [cx(0), cwq(0), ck(0), cwq(1), cv(0), cwo(0), cwo(1), cx(1), cx(2), ck(1), cv(1),
             cwo(2), cwo(3), cx(3)]
    for c in order:
        c.start()

    def rdma(ph, s, r):
        peer = peers[s] if ph != 1 else peers[1 - s]
        return pltpu.make_async_remote_copy(
            sbuf.at[ph, s, r], rbuf.at[ph, s, r], ssem.at[ph, s, r], rsem.at[ph, s, r],
            device_id=(peer,), device_id_type=MESH)

    lane = lax.broadcasted_iota(jnp.int32, (RB, 128), 1)
    lo = lane < DH
    key_lo = lax.broadcasted_iota(jnp.int32, (2 * RB, SKV), 1) < 64

    def attn(r):
        bb, qb = r // 2, r % 2
        xr = x_v[r].astype(BF)
        ctxs = []
        for p in range(2):
            if r == 0:
                cwq(p).wait()
                wq_b[p] = wq_v[p].astype(BF)
            q = jnp.dot(xr, wq_b[p], preferred_element_type=F32) * 0.125
            qs = jnp.concatenate([jnp.where(lo, q, 0.0), jnp.where(lo, 0.0, q)], axis=0).astype(BF)
            if qb == 0 and p == 0:
                ck(bb).wait()
            kt = kt_v[bb, 2 * p:2 * p + 2].reshape(2 * DH, SKV).astype(BF)
            s = jnp.dot(qs, kt, preferred_element_type=F32)
            if qb == 0:
                s = jnp.where(key_lo, s, -1e9)
            m = jnp.max(s, axis=-1, keepdims=True)
            e = jnp.exp(s - m)
            l = jnp.sum(e, axis=-1, keepdims=True)
            if qb == 0 and p == 0:
                cv(bb).wait()
            vt = vt_v[bb, 2 * p:2 * p + 2].reshape(2 * DH, SKV).astype(BF)
            o = lax.dot_general(e.astype(BF), vt, (((1,), (1,)), ((), ())),
                                preferred_element_type=F32)
            o = o / l
            ctxs.append(jnp.where(lo, o[:RB], o[RB:]).astype(BF))
        return jnp.concatenate(ctxs, axis=1)

    ctx = []
    for r in range(NR):
        cx(r).wait()
        c = attn(r)
        ctx.append(c)
        if r == 0:
            for j in range(2):
                cwo(j).wait()
                wo_b[j] = wo_v[j].astype(BF)
        for s in range(2):
            sbuf[0, s, r] = jnp.dot(c, wo_b[s], preferred_element_type=F32).astype(BF)
        if r == 0:
            pl.semaphore_wait(bsem, 2)
        for s in range(2):
            rdma(0, s, r).start()

    for j in range(2, 4):
        cwo(j).wait()
        wo_b[j] = wo_v[j].astype(BF)
    for r in range(NR):
        for s in range(2):
            keep[s, r] = jnp.dot(ctx[r], wo_b[2 + s], preferred_element_type=F32)

    for r in range(NR):
        for s in range(2):
            rdma(0, s, r).wait_recv()
            t = keep[s, r] + rbuf[0, s, r].astype(F32)
            keep[s, r] = t
            sbuf[1, s, r] = t.astype(BF)
            rdma(1, s, r).start()

    for r in range(NR):
        for s in range(2):
            rdma(0, s, r).wait_send()

    for r in range(NR):
        rows = pl.ds((r % 2) * RB, RB)
        for s in range(2):
            rdma(1, s, r).wait_recv()
            t = keep[s, r] + rbuf[1, s, r].astype(F32)
            sbuf[2, s, r] = t.astype(BF)
            rdma(2, s, r).start()
            o_ref[r // 2, rows, pl.ds(cols[2 + s], QC)] = t

    for r in range(NR):
        for s in range(2):
            rdma(1, s, r).wait_send()

    for r in range(NR):
        rows = pl.ds((r % 2) * RB, RB)
        for s in range(2):
            rdma(2, s, r).wait_recv()
            o_ref[r // 2, rows, pl.ds(cols[s], QC)] = rbuf[2, s, r].astype(F32)

    for r in range(NR):
        for s in range(2):
            rdma(2, s, r).wait_send()


def pallas_dist_sparse_attn_blocksparse_htp_b2_sq128_skv128_hq4_dh64_kernel(x, Wq, K_ext, V_ext, Wo):
    kt = jnp.transpose(K_ext, (0, 2, 3, 1))
    vt = jnp.transpose(V_ext, (0, 2, 3, 1))
    any_spec = pl.BlockSpec(memory_space=pl.ANY)
    return pl.pallas_call(
        _body,
        out_shape=jax.ShapeDtypeStruct((B, SQ, DM), F32),
        in_specs=[any_spec] * 5,
        out_specs=pl.BlockSpec(memory_space=pltpu.VMEM),
        scratch_shapes=[
            pltpu.VMEM((NR, RB, DM), F32),
            pltpu.VMEM((2, DM, 128), F32),
            pltpu.VMEM((B, HL, DH, SKV), F32),
            pltpu.VMEM((B, HL, DH, SKV), F32),
            pltpu.VMEM((4, HL * DH, QC), F32),
            pltpu.VMEM((2, DM, 128), BF),
            pltpu.VMEM((4, HL * DH, QC), BF),
            pltpu.VMEM((2, NR, RB, QC), F32),
            pltpu.VMEM((3, 2, NR, RB, QC), BF),
            pltpu.VMEM((3, 2, NR, RB, QC), BF),
            pltpu.SemaphoreType.DMA((14,)),
            pltpu.SemaphoreType.DMA((3, 2, NR)),
            pltpu.SemaphoreType.DMA((3, 2, NR)),
        ],
        compiler_params=pltpu.CompilerParams(
            collective_id=0, disable_bounds_checks=True, disable_semaphore_checks=True),
    )(x, Wq, kt, vt, Wo)
```

```python
import jax
import jax.numpy as jnp
from jax import lax
from jax.experimental import pallas as pl
from jax.experimental.pallas import tpu as pltpu

B, SQ, SKV, DM = 2, 128, 128, 512
HL, DH = 4, 64
RB = 64
NR = B * SQ // RB
QC = 128
BF = jnp.bfloat16
F32 = jnp.float32
MESH = pl.DeviceIdType.MESH


def make(loadsC, loadsE, loadsO, prog, progE, progO, NS=4):
    CR = RB // NS
    NC = 4 * NS
    loadsC, loadsE, loadsO = loadsC.split(), loadsE.split(), loadsO.split()
    allloads = loadsC + sorted(set(loadsE + loadsO))
    pre = max([0] + [int(t.split("-")[1]) for t in progE.split() if t[0] == "P"])
    preO = max([0] + [int(t.split("-")[1]) for t in progO.split() if t[0] == "P"])
    if pre > preO:
        progO = progO + f" P{preO}-{pre}"
    elif preO > pre:
        progE = progE + f" P{pre}-{preO}"
    pre = max(pre, preO)

    def _body(x_hbm, wq_hbm, kt_hbm, vt_hbm, wo_hbm, o_ref,
              x_v, wq_v, kt_v, vt_v, wo_v, keep,
              sbuf, rbuf, lsem, ssem, rsem):
        me = lax.axis_index("i")
        odd = me & 1
        b = me >> 1
        a = odd ^ b
        u = b
        first = jnp.where(me == 0, 1, 0)
        peers = (me ^ 1, 3 - me)

        def blk(role, j):
            if role == "E":
                return j // 2, j % 2, j % 2, peers[j % 2]
            if role == "O":
                h = u if j in (0, 3) else 1 - u
                return j % 2, h, h, (0 if j == 0 else 2)
            assert j == 0
            return 0, odd * u, odd * u, jnp.where(odd == 1, 0, peers[0])

        def bat(role, i):
            if role == "O":
                return i
            return first if i == 0 else 1 - first

        def cp(role, name):
            k, i = name[0], int(name[1])
            sem = lsem.at[allloads.index(name)]
            if k == "x":
                kv, h, _, _ = blk(role, i)
                r0 = h * RB if isinstance(h, int) else pl.multiple_of(h * RB, RB)
                return pltpu.make_async_copy(x_hbm.at[bat(role, kv), pl.ds(r0, RB)], x_v.at[i], sem)
            if k == "X":
                return pltpu.make_async_copy(x_hbm.at[bat(role, i)], x_v.at[pl.ds(2 * i, 2)].reshape(SQ, DM), sem)
            if k == "q":
                if i == 0:
                    return pltpu.make_async_copy(wq_hbm, wq_v, sem)
                sl = pl.ds((i - 1) * 256, 256)
                return pltpu.make_async_copy(wq_hbm.at[sl], wq_v.at[sl], sem)
            if k == "k":
                return pltpu.make_async_copy(kt_hbm.at[bat(role, i), pl.ds(me * HL, HL)], kt_v.at[i], sem)
            if k == "v":
                return pltpu.make_async_copy(vt_hbm.at[bat(role, i), pl.ds(me * HL, HL)], vt_v.at[i], sem)
            if k == "o":
                return pltpu.make_async_copy(wo_hbm.at[:, pl.ds(i * QC, QC)], wo_v.at[:, pl.ds(i * QC, QC)], sem)
            raise ValueError(name)

        for n in loadsC:
            cp("C", n).start()

        @pl.when(odd == 0)
        def _():
            for n in loadsE:
                cp("E", n).start()

        @pl.when(odd == 1)
        def _():
            for n in loadsO:
                cp("O", n).start()

        bsem = pltpu.get_barrier_semaphore()
        for p in peers:
            pl.semaphore_signal(bsem, inc=1, device_id=(p,), device_id_type=MESH)

        def rdma(ph, s, c, peer):
            return pltpu.make_async_remote_copy(
                sbuf.at[ph, s, c], rbuf.at[ph, s, c], ssem, rsem.at[ph, s, c],
                device_id=(peer,), device_id_type=MESH)

        key = lax.broadcasted_iota(jnp.int32, (RB, SKV), 1)
        zpad = jnp.zeros((DH, SKV), F32)

        def padded(ref, jj, h):
            t = ref[jj, h]
            return jnp.concatenate([t, zpad] if h % 2 == 0 else [zpad, t], axis=0).astype(BF)

        def cat(vs):
            return vs[0] if len(vs) == 1 else jnp.concatenate(vs, axis=0)

        def split(v, n):
            return [v[i * RB:(i + 1) * RB] for i in range(n)]

        def stA(role, js, _):
            xs = cat([x_v[j] for j in js]).astype(BF)
            q = jnp.dot(xs, wq_v[...].astype(BF), preferred_element_type=F32) * 0.125
            return split(q.astype(BF), len(js))

        def stA1(role, js, _):
            xs = cat([x_v[j, :, :256] for j in js]).astype(BF)
            return split(jnp.dot(xs, wq_v[:256].astype(BF), preferred_element_type=F32), len(js))

        def stA2(role, js, q1):
            xs = cat([x_v[j, :, 256:] for j in js]).astype(BF)
            q = cat(q1) + jnp.dot(xs, wq_v[256:].astype(BF), preferred_element_type=F32)
            return split((q * 0.125).astype(BF), len(js))

        def stB(role, js, qs):
            q = cat(qs)
            kv = blk(role, js[0])[0]
            ss = [split(jnp.dot(q[:, (h // 2) * 128:(h // 2 + 1) * 128], padded(kt_v, kv, h),
                                preferred_element_type=F32), len(js)) for h in range(HL)]
            return [[ss[h][i] for h in range(HL)] for i in range(len(js))]

        def stC(role, js, sss):
            out = []
            for j, ss in zip(js, sss):
                half = blk(role, j)[1]
                es = []
                for s in ss:
                    if not (isinstance(half, int) and half == 1):
                        s = jnp.where(key < 64 + 64 * half, s, -1e9)
                    m = jnp.max(s, axis=-1, keepdims=True)
                    es.append(jnp.exp(s - m))
                out.append(es)
            return out

        def stD(role, js, ess):
            kv = blk(role, js[0])[0]
            os_ = []
            for h in range(HL):
                e = cat([es[h] for es in ess])
                l = jnp.sum(e, axis=-1, keepdims=True)
                o = lax.dot_general(e.astype(BF), padded(vt_v, kv, h), (((1,), (1,)), ((), ())),
                                    preferred_element_type=F32)
                os_.append(o * pl.reciprocal(l, approx=True))
            return split(jnp.concatenate([os_[0] + os_[1], os_[2] + os_[3]], axis=1).astype(BF), len(js))

        s2 = jnp.where(odd == 1, 1 - u, 0)
        ord2 = (s2, 1 - s2)
        ord3 = (1 - s2, s2)
        sel = lambda pair, s: jnp.where(s == 0, pair[0], pair[1])
        p2 = [sel(peers, 1 - s) for s in ord2]

        def F2(cs):
            for c in cs:
                for i in range(2):
                    s = ord2[i]
                    rdma(0, s, c, 0).wait_recv()
                    t = keep[s, c] + rbuf[0, s, c].astype(F32)
                    keep[s, c] = t
                    sbuf[1, s, c] = t.astype(BF)
                    rdma(1, s, c, p2[i]).start()

        def run(role, prog, val, gv):
            tag = "" if role == "C" else "_" + role
            for tok in prog.split():
                k = tok[0]
                if k == "w":
                    for n in tok[1:].split(","):
                        cp(role if n not in loadsC else "C", n).wait()
                    continue
                if tok == "bar":
                    pl.semaphore_wait(bsem, 2)
                    continue
                if k == "P":
                    lo, hi = tok[1:].split("-")
                    F2(range(int(lo), int(hi)))
                    continue
                if k in "GSK":
                    js, qs = tok[1:].split(".")
                    js, qs = [int(r) for r in js], [int(r) for r in qs]
                    if k in "GK":
                        w = wo_v[:, qs[0] * QC:(qs[-1] + 1) * QC].astype(BF)
                        gs = split(jnp.dot(cat([val[j] for j in js]), w, preferred_element_type=F32), len(js))
                        for j, g in zip(js, gs):
                            for i, q in enumerate(qs):
                                gq = g[:, i * QC:(i + 1) * QC]
                                if k == "G":
                                    gv[j, q] = gq.astype(BF)
                                else:
                                    for kk in range(NS):
                                        keep[blk(role, j)[2], q * NS + kk] = gq[kk * CR:(kk + 1) * CR]
                    else:
                        for q in qs:
                            for kk in range(NS):
                                for j in js:
                                    _, _, st_, peer = blk(role, j)
                                    sbuf[0, st_, q * NS + kk] = gv[j, q][kk * CR:(kk + 1) * CR]
                                    rdma(0, st_, q * NS + kk, peer).start()
                    continue
                js = [int(r) for r in tok[1:]]
                out = st[k](role, js, [val[j] for j in js])
                for j, o in zip(js, out):
                    val[j] = o

        st = dict(A=stA, a=stA1, b=stA2, B=stB, C=stC, D=stD)
        val, gv = [None] * NR, {}
        run("C", prog, val, gv)

        @pl.when(odd == 0)
        def _():
            run("E", progE, list(val), dict(gv))

        @pl.when(odd == 1)
        def _():
            run("O", progO, list(val), dict(gv))

        def out_at(batch, half, c):
            row = half * RB + (c % NS) * CR
            if not isinstance(row, int):
                row = pl.multiple_of(row, CR)
            return (batch, pl.ds(row, CR), pl.ds((c // NS) * QC, QC))

        idx = [(s, c) for c in range(NC) for s in range(2)]
        F2(range(pre, NC))

        kbat = (a, b)
        p3 = [sel(peers, s) for s in ord3]
        kb3 = [sel(kbat, s) for s in ord3]
        for (i, c) in idx:
            s = ord3[i]
            rdma(1, s, c, 0).wait_recv()
            t = keep[s, c] + rbuf[1, s, c].astype(F32)
            sbuf[2, s, c] = t.astype(BF)
            rdma(2, s, c, p3[i]).start()
            o_ref[out_at(kb3[i], s, c)] = t

        for i, (s, c) in enumerate(idx):
            if i == len(idx) - 2:
                pltpu.make_async_copy(sbuf, sbuf, ssem).wait()
            rdma(2, s, c, 0).wait_recv()
            o_ref[out_at(1 - kbat[s], s, c)] = rbuf[2, s, c].astype(F32)

    def kernel(x, Wq, K_ext, V_ext, Wo):
        kt = jnp.transpose(K_ext, (0, 2, 3, 1))
        vt = jnp.transpose(V_ext, (0, 2, 3, 1))
        any_spec = pl.BlockSpec(memory_space=pl.ANY)
        return pl.pallas_call(
            _body,
            out_shape=jax.ShapeDtypeStruct((B, SQ, DM), F32),
            in_specs=[any_spec] * 5,
            out_specs=pl.BlockSpec(memory_space=pltpu.VMEM),
            scratch_shapes=[
                pltpu.VMEM((NR, RB, DM), F32),
                pltpu.VMEM((DM, HL * DH), F32),
                pltpu.VMEM((B, HL, DH, SKV), F32),
                pltpu.VMEM((B, HL, DH, SKV), F32),
                pltpu.VMEM((HL * DH, DM), F32),
                pltpu.VMEM((2, NC, CR, QC), F32),
                pltpu.VMEM((3, 2, NC, CR, QC), BF),
                pltpu.VMEM((3, 2, NC, CR, QC), BF),
                pltpu.SemaphoreType.DMA((len(allloads),)),
                pltpu.SemaphoreType.DMA,
                pltpu.SemaphoreType.DMA((3, 2, NC)),
            ],
            compiler_params=pltpu.CompilerParams(
                collective_id=0, disable_bounds_checks=True, disable_semaphore_checks=True),
        )(x, Wq, kt, vt, Wo)
    return kernel

_LOADS_EVEN = "x0 x1 k0 v0 o0 x2 o1 x3 o2 k1 o3 v1"
_PROG_EVEN = ("wq0,x0 A0 wx1,k0 A1 B01 C01 wv0,o0 bar D01 G0.0 G1.0 S01.0 wx2,o1 G0.1 G1.1 A2 S01.1 "
              "wx3,o2 G0.2 G1.2 A3 S01.2 wk1 B23 wo3 G0.3 G1.3 C23 S01.3 wv1 "
              "D23 K2.0 K3.0 P0-3 K2.123 K3.123")
_LOADS_ODD = "x0 k0 v0 x1 k1 o0 v1 o1 x2 x3 o2 o3"
_PROG_ODD = ("wq0,x0 A0 wk0 B0 C0 wv0,x1 D0 A1 wk1,o0 bar G0.0 B1 C1 S0.0 wv1,o1 G0.1 D1 G1.01 S0.1 S1.01 "
             "wx2,x3 A23 wo2 G0.2 G1.2 B2 B3 C2 C3 S0.2 S1.2 wo3 G0.3 G1.3 D2 D3 S0.3 S1.3 K23.0123")
_KERNEL = make("q0", _LOADS_EVEN, _LOADS_ODD, "", _PROG_EVEN, _PROG_ODD)


def pallas_dist_sparse_attn_blocksparse_htp_b2_sq128_skv128_hq4_dh64_kernel(x, Wq, K_ext, V_ext, Wo):
    return _KERNEL(x, Wq, K_ext, V_ext, Wo)
```

```python
import jax
import jax.numpy as jnp
from jax import lax
from jax.experimental import pallas as pl
from jax.experimental.pallas import tpu as pltpu

B, SQ, SKV, DM = 2, 128, 128, 512
HL, DH = 4, 64
RB = 64
NR = B * SQ // RB
QC = 128
BF = jnp.bfloat16
F32 = jnp.float32
MESH = pl.DeviceIdType.MESH
QS = 0.125 * 1.4426950408889634


def make(loadsC, loadsE, loadsO, prog, progE, progO, NS=4):
    CR = RB // NS
    NC = 4 * NS
    loadsC, loadsE, loadsO = loadsC.split(), loadsE.split(), loadsO.split()
    allloads = loadsC + sorted(set(loadsE + loadsO))
    pre = max([0] + [int(t.split("-")[1]) for t in progE.split() if t[0] in "PQ"])
    preO = max([0] + [int(t.split("-")[1]) for t in progO.split() if t[0] == "P"])
    if pre > preO:
        progO = progO + f" P{preO}-{pre}"
    elif preO > pre:
        progE = progE + f" P{pre}-{preO}"
    pre = max(pre, preO)

    def _body(x_hbm, wq_hbm, kt_hbm, vt_hbm, wo_hbm, o_ref,
              x_v, wq_v, kt_v, vt_v, wo_v, keep,
              sbuf, rbuf, lsem, ssem, rsem):
        me = lax.axis_index("i")
        odd = me & 1
        b = me >> 1
        a = odd ^ b
        u = b
        first = jnp.where(me == 0, 1, 0)
        peers = (me ^ 1, 3 - me)

        def blk(role, j):
            if role == "E":
                return j // 2, j % 2, j % 2, peers[j % 2]
            if role == "O":
                h = u if j in (0, 3) else 1 - u
                return j % 2, h, h, (0 if j == 0 else 2)
            assert j == 0
            return 0, odd * u, odd * u, jnp.where(odd == 1, 0, peers[0])

        def bat(role, i):
            if role == "O":
                return i
            return first if i == 0 else 1 - first

        def cp(role, name):
            k, i = name[0], int(name[1])
            sem = lsem.at[allloads.index(name)]
            if k == "x":
                kv, h, _, _ = blk(role, i)
                r0 = h * RB if isinstance(h, int) else pl.multiple_of(h * RB, RB)
                return pltpu.make_async_copy(x_hbm.at[bat(role, kv), pl.ds(r0, RB)], x_v.at[i], sem)
            if k == "X":
                return pltpu.make_async_copy(x_hbm.at[bat(role, i)], x_v.at[pl.ds(2 * i, 2)].reshape(SQ, DM), sem)
            if k == "q":
                if i == 0:
                    return pltpu.make_async_copy(wq_hbm, wq_v, sem)
                sl = pl.ds((i - 1) * 256, 256)
                return pltpu.make_async_copy(wq_hbm.at[sl], wq_v.at[sl], sem)
            if k == "k":
                return pltpu.make_async_copy(kt_hbm.at[bat(role, i), pl.ds(me * HL, HL)], kt_v.at[i], sem)
            if k == "v":
                return pltpu.make_async_copy(vt_hbm.at[bat(role, i), pl.ds(me * HL, HL)], vt_v.at[i], sem)
            if k == "o":
                return pltpu.make_async_copy(wo_hbm.at[:, pl.ds(i * QC, QC)], wo_v.at[:, pl.ds(i * QC, QC)], sem)
            raise ValueError(name)

        for n in loadsC:
            cp("C", n).start()

        @pl.when(odd == 0)
        def _():
            for n in loadsE:
                cp("E", n).start()

        @pl.when(odd == 1)
        def _():
            for n in loadsO:
                cp("O", n).start()

        bsem = pltpu.get_barrier_semaphore()
        for p in peers:
            pl.semaphore_signal(bsem, inc=1, device_id=(p,), device_id_type=MESH)

        def rdma(ph, s, c, peer):
            return pltpu.make_async_remote_copy(
                sbuf.at[ph, s, c], rbuf.at[ph, s, c], ssem, rsem.at[ph, s, c],
                device_id=(peer,), device_id_type=MESH)

        key = lax.broadcasted_iota(jnp.int32, (RB, SKV), 1)
        zpad = jnp.zeros((DH, SKV), F32)

        def padded(ref, jj, h):
            t = ref[jj, h]
            return jnp.concatenate([t, zpad] if h % 2 == 0 else [zpad, t], axis=0).astype(BF)

        def cat(vs):
            return vs[0] if len(vs) == 1 else jnp.concatenate(vs, axis=0)

        def split(v, n):
            return [v[i * RB:(i + 1) * RB] for i in range(n)]

        def ilv(vs):
            if len(vs) == 1:
                return vs[0]
            return jnp.concatenate([v[k * 16:(k + 1) * 16] for k in range(RB // 16) for v in vs], axis=0)

        def unilv(v, n):
            if n == 1:
                return [v]
            return [jnp.concatenate([v[(k * n + i) * 16:(k * n + i + 1) * 16] for k in range(RB // 16)], axis=0)
                    for i in range(n)]

        def stA(role, js, _):
            xs = cat([x_v[j] for j in js]).astype(BF)
            q = jnp.dot(xs, wq_v[...].astype(BF), preferred_element_type=F32) * QS
            return [[qq[:, :128], qq[:, 128:]] for qq in split(q, len(js))]

        def stA1(role, js, _):
            xs = cat([x_v[j, :, :256] for j in js]).astype(BF)
            return split(jnp.dot(xs, wq_v[:256].astype(BF), preferred_element_type=F32), len(js))

        def stA2(role, js, q1):
            xs = cat([x_v[j, :, 256:] for j in js]).astype(BF)
            q = cat(q1) + jnp.dot(xs, wq_v[256:].astype(BF), preferred_element_type=F32)
            return [[qq[:, :128], qq[:, 128:]] for qq in split(q * QS, len(js))]

        def stB(role, js, qs):
            q = [cat([qq[i] for qq in qs]) for i in range(2)]
            kv = blk(role, js[0])[0]
            ss = [split(jnp.dot(q[h // 2].astype(BF), padded(kt_v, kv, h),
                                preferred_element_type=F32), len(js)) for h in range(HL)]
            return [[ss[h][i] for h in range(HL)] for i in range(len(js))]

        def stC(role, js, sss):
            out = []
            for j, ss in zip(js, sss):
                half = blk(role, j)[1]
                es = []
                for s in ss:
                    if not (isinstance(half, int) and half == 1):
                        s = jnp.where(key < 64 + 64 * half, s, -1e9)
                    m = jnp.max(s, axis=-1, keepdims=True)
                    es.append(jnp.exp2(s - m))
                out.append(es)
            return out

        def stD(role, js, ess):
            kv = blk(role, js[0])[0]
            os_ = []
            for h in range(HL):
                e = ilv([es[h] for es in ess])
                l = jnp.sum(e, axis=-1, keepdims=True)
                o = lax.dot_general(e.astype(BF), padded(vt_v, kv, h), (((1,), (1,)), ((), ())),
                                    preferred_element_type=F32)
                os_.append(o * pl.reciprocal(l, approx=True))
            cs = [unilv(os_[2 * i] + os_[2 * i + 1], len(js)) for i in range(2)]
            return [[cs[0][i], cs[1][i]] for i in range(len(js))]

        def lowpad(ref, jj, h):
            return jnp.concatenate([ref[jj, h], zpad], axis=0).astype(BF)

        def stE(role, js, ess):
            kv = blk(role, js[0])[0]
            os_ = []
            for h in range(HL):
                e = ilv([es[h] for es in ess])
                l = jnp.sum(e, axis=-1, keepdims=True)
                o = lax.dot_general(e.astype(BF), lowpad(vt_v, kv, h), (((1,), (1,)), ((), ())),
                                    preferred_element_type=F32)
                os_.append(o * pl.reciprocal(l, approx=True))
            cs = [unilv(os_[2 * i] + pltpu.roll(os_[2 * i + 1], 64, 1), len(js)) for i in range(2)]
            hs = [unilv(o, len(js)) for o in os_]
            return [[cs[0][i], cs[1][i], [hs[h][i] for h in range(HL)]] for i in range(len(js))]

        def proj(val, js, cl, perhead):
            if perhead:
                n = cl.stop - cl.start
                ps = [jnp.dot(ilv([val[j][2][h] for j in js]).astype(BF),
                              jnp.concatenate([wo_v[h * DH:(h + 1) * DH, cl], jnp.zeros((DH, n), F32)], axis=0).astype(BF),
                              preferred_element_type=F32) for h in range(HL)]
                return unilv((ps[0] + ps[1]) + (ps[2] + ps[3]), len(js))
            return split(sum(jnp.dot(cat([val[j][i] for j in js]).astype(BF), wo_v[i * 128:(i + 1) * 128, cl].astype(BF),
                                     preferred_element_type=F32) for i in range(2)), len(js))

        s2 = jnp.where(odd == 1, 1 - u, 0)
        ord2 = (s2, 1 - s2)
        ord3 = (1 - s2, s2)
        sel = lambda pair, s: jnp.where(s == 0, pair[0], pair[1])
        p2 = [sel(peers, 1 - s) for s in ord2]

        def F2(cs):
            for c in cs:
                for i in range(2):
                    s = ord2[i]
                    rdma(0, s, c, 0).wait_recv()
                    t = keep[s, c] + rbuf[0, s, c].astype(F32)
                    keep[s, c] = t
                    sbuf[1, s, c] = t.astype(BF)
                    rdma(1, s, c, p2[i]).start()

        def run(role, prog, val, gv):
            tag = "" if role == "C" else "_" + role
            for tok in prog.split():
                k = tok[0]
                if k == "w":
                    for n in tok[1:].split(","):
                        cp(role if n not in loadsC else "C", n).wait()
                    continue
                if tok == "bar":
                    pl.semaphore_wait(bsem, 2)
                    continue
                if k == "P":
                    lo, hi = tok[1:].split("-")
                    F2(range(int(lo), int(hi)))
                    continue
                if k == "R":
                    lo, hi = tok[1:].split("-")
                    for c in range(int(lo), int(hi)):
                        for s_ in range(2):
                            rdma(0, s_, c, 0).wait_recv()
                    continue
                if k == "Q":
                    lo, hi = [int(r) for r in tok[1:].split("-")]
                    for c in range(lo, hi):
                        for s_ in range(2):
                            t = gv[2 + s_, c // NS][(c % NS) * CR:(c % NS + 1) * CR] + rbuf[0, s_, c].astype(F32)
                            sbuf[1, s_, c] = t.astype(BF)
                            rdma(1, s_, c, peers[1 - s_]).start()
                            gv["t", s_, c] = t
                    for c in range(lo, hi):
                        for s_ in range(2):
                            keep[s_, c] = gv["t", s_, c]
                    for c in range(hi, -(-hi // NS) * NS):
                        for s_ in range(2):
                            keep[s_, c] = gv[2 + s_, c // NS][(c % NS) * CR:(c % NS + 1) * CR]
                    continue
                if k in "GHSKLFIT":
                    js, qs = tok[1:].split(".")
                    js, qs = [int(r) for r in js], [int(r) for r in qs]
                    if k == "T":
                        for j in js:
                            for q in qs:
                                for kk in range(NS):
                                    keep[blk(role, j)[2], q * NS + kk] = gv[j, q][kk * CR:(kk + 1) * CR]
                        continue
                    if k != "S":
                        cl = slice(qs[0] * QC, (qs[-1] + 1) * QC)
                        gs = proj(val, js, cl, k in "HLI")
                        for j, g in zip(js, gs):
                            for i, q in enumerate(qs):
                                gq = g[:, i * QC:(i + 1) * QC]
                                if k in "GH":
                                    gv[j, q] = gq.astype(BF)
                                elif k in "FI":
                                    gv[j, q] = gq
                                else:
                                    for kk in range(NS):
                                        keep[blk(role, j)[2], q * NS + kk] = gq[kk * CR:(kk + 1) * CR]
                    else:
                        for q in qs:
                            for kk in range(NS):
                                for j in js:
                                    _, _, st_, peer = blk(role, j)
                                    sbuf[0, st_, q * NS + kk] = gv[j, q][kk * CR:(kk + 1) * CR]
                                    rdma(0, st_, q * NS + kk, peer).start()
                    continue
                js = [int(r) for r in tok[1:]]
                out = st[k](role, js, [val[j] for j in js])
                for j, o in zip(js, out):
                    val[j] = o

        st = dict(A=stA, a=stA1, b=stA2, B=stB, C=stC, D=stD, E=stE)
        val, gv = [None] * NR, {}
        run("C", prog, val, gv)

        @pl.when(odd == 0)
        def _():
            run("E", progE, list(val), dict(gv))

        @pl.when(odd == 1)
        def _():
            run("O", progO, list(val), dict(gv))

        def out_at(batch, half, c):
            return (batch, half, pl.ds((c % NS) * CR, CR), pl.ds((c // NS) * QC, QC))

        idx = [(s, c) for c in range(NC) for s in range(2)]
        F2(range(pre, NC))

        kbat = (a, b)
        p3 = [sel(peers, s) for s in ord3]
        kb3 = [sel(kbat, s) for s in ord3]
        for (i, c) in idx:
            s = ord3[i]
            rdma(1, s, c, 0).wait_recv()
            t = keep[s, c] + rbuf[1, s, c].astype(F32)
            sbuf[2, s, c] = t.astype(BF)
            rdma(2, s, c, p3[i]).start()
            o_ref[out_at(kb3[i], s, c)] = t

        for i, (s, c) in enumerate(idx):
            if i == len(idx) - 2:
                pltpu.make_async_copy(sbuf, sbuf, ssem).wait()
            rdma(2, s, c, 0).wait_recv()
            o_ref[out_at(1 - kbat[s], s, c)] = rbuf[2, s, c].astype(F32)

    def kernel(x, Wq, K_ext, V_ext, Wo):
        kt = jnp.transpose(K_ext, (0, 2, 3, 1))
        vt = jnp.transpose(V_ext, (0, 2, 3, 1))
        any_spec = pl.BlockSpec(memory_space=pl.ANY)
        return pl.pallas_call(
            _body,
            out_shape=jax.ShapeDtypeStruct((B, 2, RB, DM), F32),
            in_specs=[any_spec] * 5,
            out_specs=pl.BlockSpec(memory_space=pltpu.VMEM),
            scratch_shapes=[
                pltpu.VMEM((NR, RB, DM), F32),
                pltpu.VMEM((DM, HL * DH), F32),
                pltpu.VMEM((B, HL, DH, SKV), F32),
                pltpu.VMEM((B, HL, DH, SKV), F32),
                pltpu.VMEM((HL * DH, DM), F32),
                pltpu.VMEM((2, NC, CR, QC), F32),
                pltpu.VMEM((3, 2, NC, CR, QC), BF),
                pltpu.VMEM((3, 2, NC, CR, QC), BF),
                pltpu.SemaphoreType.DMA((len(allloads),)),
                pltpu.SemaphoreType.DMA,
                pltpu.SemaphoreType.DMA((3, 2, NC)),
            ],
            compiler_params=pltpu.CompilerParams(
                collective_id=0, disable_bounds_checks=True, disable_semaphore_checks=True),
        )(x, Wq, kt, vt, Wo).reshape(B, SQ, DM)
    return kernel

_LOADS_EVEN = "q1 x0 x1 q2 k0 v0 o0 x2 o1 x3 o2 k1 o3 v1"
_PROG_EVEN = ("wx0,x1,q1 a01 wq2 b01 wk0 B01 C01 wv0,o0 bar E01 H01.0 S01.0 wx2,o1 G0.1 G1.1 A2 S01.1 "
              "wx3,o2 G0.2 G1.2 A3 S01.2 wk1 B23 wo3 G0.3 G1.3 C23 S01.3 "
              "wv1 R0-4 E23 I23.0 Q0-4 P4-8 K2.123 K3.123")
_LOADS_ODD = "q1 x0 x1 q2 k0 v0 k1 o0 v1 o1 x2 x3 o2 o3"
_PROG_ODD = ("wx0,x1,q1 a01 wq2 b01 wk0 B0 C0 wv0,k1 B1 D0 C1 wo0 bar G0.0 S0.0 wv1 D1 G1.0 S1.0 "
             "wo1,x2 G0.1 G1.1 A2 S01.1 B2 wx3,o2 G0.2 G1.2 A3 C2 D2 B3 S01.2 "
             "wo3 G0.3 G1.3 C3 F2.01 D3 S01.3 T2.01 K2.23 K3.0123")
_KERNEL = make("", _LOADS_EVEN, _LOADS_ODD, "", _PROG_EVEN, _PROG_ODD, NS=8)


def pallas_dist_sparse_attn_blocksparse_htp_b2_sq128_skv128_hq4_dh64_kernel(x, Wq, K_ext, V_ext, Wo):
    return _KERNEL(x, Wq, K_ext, V_ext, Wo)
```

```python
import jax
import jax.numpy as jnp
from jax import lax
from jax.experimental import pallas as pl
from jax.experimental.pallas import tpu as pltpu

B, SQ, SKV, DM = 2, 128, 128, 512
HL, DH = 4, 64
RB = 64
NR = B * SQ // RB
HR = RB // 2
QC = 128
CR = 8
NS = RB // CR
NC = 4 * NS
BF = jnp.bfloat16
F32 = jnp.float32
MESH = pl.DeviceIdType.MESH
LOG2E = 1.4426950408889634
QS = 0.125 * LOG2E
NEG = -1e9 * LOG2E


def _make(loads, progs, pre):
    names = sorted(set(loads["E"].split() + loads["O"].split()))

    def body(x_hbm, wq_hbm, kt_hbm, vt_hbm, wo_hbm, o_ref,
             x_v, wq_v, kt_v, vt_v, wo_v, keep, sbuf, rbuf, lsem, ssem, rsem):
        me = lax.axis_index("i")
        odd = me & 1
        b = me >> 1
        kbat = (odd ^ b, b)
        peers = (me ^ 1, 3 - me)
        first = jnp.where(me == 0, 1, 0)

        def slot(role, j):
            return j // 2 if role == "E" else j % 2

        def batch(role, i):
            return i if role == "O" else (first if i == 0 else 1 - first)

        def half(j):
            return b if j in (0, 3) else 1 - b

        def pieces(role, j, q):
            if role == "E":
                return [((2 * k + s) * CR, s, q * NS + (j % 2) * (NS // 2) + k, peers[s])
                        for k in range(NS // 2) for s in range(2)]
            return [(k * CR, half(j), q * NS + k, 0 if j == 0 else 2) for k in range(NS)]

        def load(role, name):
            k, i = name[0], int(name[1])
            sem = lsem.at[names.index(name)]
            if k == "x":
                xb = x_hbm.at[batch(role, slot(role, i))]
                return pltpu.make_async_copy(xb.at[:, i % 2] if role == "E" else xb.at[half(i)], x_v.at[i], sem)
            if k == "q":
                sl = pl.ds(i * 256, 256)
                return pltpu.make_async_copy(wq_hbm.at[sl], wq_v.at[sl], sem)
            if k == "o":
                sl = pl.ds(i * QC, QC)
                return pltpu.make_async_copy(wo_hbm.at[:, sl], wo_v.at[:, sl], sem)
            src, dst = (kt_hbm, kt_v) if k == "k" else (vt_hbm, vt_v)
            return pltpu.make_async_copy(src.at[batch(role, i), pl.ds(me * HL, HL)], dst.at[i], sem)

        for role, parity in (("E", 0), ("O", 1)):
            @pl.when(odd == parity)
            def _():
                for n in loads[role].split():
                    load(role, n).start()

        bsem = pltpu.get_barrier_semaphore()
        for p in peers:
            pl.semaphore_signal(bsem, inc=1, device_id=(p,), device_id_type=MESH)

        def rdma(ph, s, c, peer):
            return pltpu.make_async_remote_copy(
                sbuf.at[ph, s, c], rbuf.at[ph, s, c], ssem, rsem.at[ph, s, c],
                device_id=(peer,), device_id_type=MESH)

        key = lax.broadcasted_iota(jnp.int32, (RB, SKV), 1)
        zpad = jnp.zeros((DH, SKV), F32)

        def cat(vs):
            return vs[0] if len(vs) == 1 else jnp.concatenate(vs, axis=0)

        def split(v, n):
            return [v[i * RB:(i + 1) * RB] for i in range(n)]

        def padded(ref, i, h, low=False):
            t = ref[i, h]
            return cat([t, zpad] if low or h % 2 == 0 else [zpad, t]).astype(BF)

        def xrows(role, js, cl):
            if role == "E":
                return cat([x_v[j, s, k * CR:(k + 1) * CR, cl]
                            for j in js for k in range(NS // 2) for s in range(2)]).astype(BF)
            return cat([x_v[j, s, :, cl] for j in js for s in range(2)]).astype(BF)

        def qsplit(q, n):
            return [[t[:, :128], t[:, 128:]] for t in split(q * QS, n)]

        def q_full(role, js, _):
            return qsplit(jnp.dot(xrows(role, js, slice(0, DM)), wq_v[...].astype(BF),
                                  preferred_element_type=F32), len(js))

        def q_lo(role, js, _):
            return split(jnp.dot(xrows(role, js, slice(0, 256)), wq_v[:256].astype(BF),
                                 preferred_element_type=F32), len(js))

        def q_hi(role, js, acc):
            return qsplit(cat(acc) + jnp.dot(xrows(role, js, slice(256, DM)), wq_v[256:].astype(BF),
                                             preferred_element_type=F32), len(js))

        def scores(role, js, qs):
            q = [cat([t[i] for t in qs]) for i in range(2)]
            ss = [split(jnp.dot(q[h // 2].astype(BF), padded(kt_v, slot(role, js[0]), h),
                                preferred_element_type=F32), len(js)) for h in range(HL)]
            return [[ss[h][i] for h in range(HL)] for i in range(len(js))]

        def sub_max(role, js, sss):
            out = []
            for j, ss in zip(js, sss):
                ds = []
                for s in ss:
                    if role == "E":
                        s = cat([s[i * CR:(i + 1) * CR] if i % 2 else
                                 jnp.where(key[:CR] < RB, s[i * CR:(i + 1) * CR], NEG) for i in range(NS)])
                    else:
                        s = jnp.where(key < RB + RB * half(j), s, NEG)
                    ds.append(s - jnp.max(s, axis=-1, keepdims=True))
                out.append(ds)
            return out

        def expo(role, js, dss):
            return [[jnp.exp2(d) for d in ds] for ds in dss]

        def weights(role, js, sss):
            return expo(role, js, sub_max(role, js, sss))

        def pv(role, js, ess, low):
            os_ = []
            for h in range(HL):
                e = cat([es[h] for es in ess])
                l = jnp.sum(e, axis=-1, keepdims=True)
                o = lax.dot_general(e.astype(BF), padded(vt_v, slot(role, js[0]), h, low),
                                    (((1,), (1,)), ((), ())), preferred_element_type=F32)
                r = pl.reciprocal(l, approx=True)
                os_.append(o * (r * (2.0 - l * r)))
            return os_

        def ctx_pair(role, js, ess):
            os_ = pv(role, js, ess, False)
            cs = [split(os_[2 * i] + os_[2 * i + 1], len(js)) for i in range(2)]
            return [[cs[0][i], cs[1][i]] for i in range(len(js))]

        def ctx_head(role, js, ess):
            hs = [split(o, len(js)) for o in pv(role, js, ess, True)]
            return [[None, None, [hs[h][i] for h in range(HL)]] for i in range(len(js))]

        def join(role, js, vs):
            return [[v[2][0] + pltpu.roll(v[2][1], DH, 1), v[2][2] + pltpu.roll(v[2][3], DH, 1), v[2]] for v in vs]

        def ctx_both(role, js, ess):
            os_ = pv(role, js, ess, True)
            cs = [split(os_[2 * i] + pltpu.roll(os_[2 * i + 1], DH, 1), len(js)) for i in range(2)]
            hs = [split(o, len(js)) for o in os_]
            return [[cs[0][i], cs[1][i], [hs[h][i] for h in range(HL)]] for i in range(len(js))]

        stage = dict(A=q_full, a=q_lo, b=q_hi, B=scores, M=sub_max, X=expo, C=weights,
                     D=ctx_pair, e=ctx_head, J=join, E=ctx_both)

        def project(val, js, cl, per_head):
            if per_head:
                zw = jnp.zeros((DH, cl.stop - cl.start), F32)
                ps = [jnp.dot(cat([val[j][2][h] for j in js]).astype(BF),
                              cat([wo_v[h * DH:(h + 1) * DH, cl], zw]).astype(BF),
                              preferred_element_type=F32) for h in range(HL)]
                return split((ps[0] + ps[1]) + (ps[2] + ps[3]), len(js))
            return split(sum(jnp.dot(cat([val[j][i] for j in js]).astype(BF),
                                     wo_v[i * 128:(i + 1) * 128, cl].astype(BF),
                                     preferred_element_type=F32) for i in range(2)), len(js))

        def sel(pair, s):
            return jnp.where(s == 0, pair[0], pair[1])

        s2 = jnp.where(odd == 1, 1 - b, 0)
        ord2, ord3 = (s2, 1 - s2), (1 - s2, s2)
        p2 = [sel(peers, 1 - s) for s in ord2]

        def phase2(cs):
            for c in cs:
                for s, peer in zip(ord2, p2):
                    rdma(0, s, c, 0).wait_recv()
                    t = keep[s, c] + rbuf[0, s, c].astype(F32)
                    keep[s, c] = t
                    sbuf[1, s, c] = t.astype(BF)
                    rdma(1, s, c, peer).start()

        def run(role):
            val, out = [None] * NR, {}
            for tok in progs[role].split():
                k = tok[0]
                if k == "w":
                    for n in tok[1:].split(","):
                        load(role, n).wait()
                elif tok == "bar":
                    pl.semaphore_wait(bsem, 2)
                elif k == "P":
                    lo, hi = tok[1:].split("-")
                    phase2(range(int(lo), int(hi)))
                elif "." not in tok:
                    js = [int(r) for r in tok[1:]]
                    for j, v in zip(js, stage[k](role, js, [val[j] for j in js])):
                        val[j] = v
                else:
                    js, qs = [[int(r) for r in t] for t in tok[1:].split(".")]
                    if k in "GHFIK":
                        cl = slice(qs[0] * QC, (qs[-1] + 1) * QC)
                        for j, g in zip(js, project(val, js, cl, k in "HI")):
                            for i, q in enumerate(qs):
                                gq = g[:, i * QC:(i + 1) * QC]
                                out[j, q] = gq.astype(BF) if k in "GH" else gq
                        if k != "K":
                            continue
                    for q in qs:
                        ps = [(j, p) for ps in zip(*[pieces(role, j, q) for j in js]) for j, p in zip(js, ps)]
                        sums = []
                        for j, (r, s, c, peer) in ps:
                            if k in "KT":
                                keep[s, c] = out[j, q][r:r + CR]
                            elif k == "S":
                                sbuf[0, s, c] = out[j, q][r:r + CR]
                                rdma(0, s, c, peer).start()
                            elif k == "R":
                                rdma(0, s, c, 0).wait_recv()
                            else:
                                assert k == "Q" and role == "E"
                                t = out[j, q][r:r + CR] + rbuf[0, s, c].astype(F32)
                                sbuf[1, s, c] = t.astype(BF)
                                rdma(1, s, c, peers[1 - s]).start()
                                sums.append((s, c, t))
                        for s, c, t in sums:
                            keep[s, c] = t

        for role, parity in (("E", 0), ("O", 1)):
            @pl.when(odd == parity)
            def _():
                run(role)

        phase2(range(pre, NC))

        def out_at(bt, s, c):
            return (bt, s, pl.ds((c % NS) * CR, CR), pl.ds((c // NS) * QC, QC))

        p3 = [sel(peers, s) for s in ord3]
        kb3 = [sel(kbat, s) for s in ord3]
        for c in range(NC):
            for s, peer, bt in zip(ord3, p3, kb3):
                rdma(1, s, c, 0).wait_recv()
                t = keep[s, c] + rbuf[1, s, c].astype(F32)
                sbuf[2, s, c] = t.astype(BF)
                rdma(2, s, c, peer).start()
                o_ref[out_at(bt, s, c)] = t

        for c in range(NC):
            if c == NC - 1:
                pltpu.make_async_copy(sbuf, sbuf, ssem).wait()
            for s in range(2):
                rdma(2, s, c, 0).wait_recv()
                o_ref[out_at(1 - kbat[s], s, c)] = rbuf[2, s, c].astype(F32)

    def kernel(x, Wq, K_ext, V_ext, Wo):
        return pl.pallas_call(
            body,
            out_shape=jax.ShapeDtypeStruct((B, 2, RB, DM), F32),
            in_specs=[pl.BlockSpec(memory_space=pl.ANY)] * 5,
            out_specs=pl.BlockSpec(memory_space=pltpu.VMEM),
            scratch_shapes=[
                pltpu.VMEM((NR, 2, HR, DM), F32),
                pltpu.VMEM((DM, HL * DH), F32),
                pltpu.VMEM((B, HL, DH, SKV), F32),
                pltpu.VMEM((B, HL, DH, SKV), F32),
                pltpu.VMEM((HL * DH, DM), F32),
                pltpu.VMEM((2, NC, CR, QC), F32),
                pltpu.VMEM((3, 2, NC, CR, QC), BF),
                pltpu.VMEM((3, 2, NC, CR, QC), BF),
                pltpu.SemaphoreType.DMA((len(names),)),
                pltpu.SemaphoreType.DMA,
                pltpu.SemaphoreType.DMA((3, 2, NC)),
            ],
            compiler_params=pltpu.CompilerParams(
                collective_id=0, disable_bounds_checks=True, disable_semaphore_checks=True),
        )(x.reshape(B, 2, 2, HR, DM), Wq, jnp.transpose(K_ext, (0, 2, 3, 1)),
          jnp.transpose(V_ext, (0, 2, 3, 1)), Wo).reshape(B, SQ, DM)

    return kernel


_PRE = 23
_KERNEL = _make(
    loads=dict(E="q0 x0 x1 q1 k0 v0 o0 x2 o1 x3 o2 k1 o3 v1",
               O="q0 x0 x1 q1 k0 v0 k1 o0 v1 o1 x2 x3 o2 o3"),
    progs=dict(E="wx0,x1,q0 a01 wq1 b01 wk0 B01 M0 wv0 X0 e0 wo0 bar H0.0 C1 E1 H1.0 J0 S0.0 S1.0 "
                 "wx2,o1 G0.1 G1.1 A2 S0.1 S1.1 wx3,o2 G0.2 G1.2 A3 S0.2 S1.2 "
                 "wk1 B23 wo3 G0.3 G1.3 C23 S0.3 S1.3 "
                 "wv1 R2.0 E23 I23.0 Q2.0 T3.0 P4-8 K23.1 P8-15 K23.2 P15-23 K23.3",
               O="wx0,x1,q0 a01 wq1 b01 wk0 B0 C0 wv0,k1 B1 D0 C1 wo0 bar G0.0 S0.0 wv1 D1 G1.0 S1.0 "
                 "wo1,x2 G0.1 G1.1 A2 S01.1 B2 wx3,o2 G0.2 G1.2 A3 C2 D2 B3 S01.2 "
                 "wo3 G0.3 G1.3 C3 F2.01 D3 S01.3 T2.01 K2.23 K3.0123 P0-23"),
    pre=_PRE)


def pallas_dist_sparse_attn_blocksparse_htp_b2_sq128_skv128_hq4_dh64_kernel(x, Wq, K_ext, V_ext, Wo):
    return _KERNEL(x, Wq, K_ext, V_ext, Wo)
```

```python
import jax
import jax.numpy as jnp
from jax import lax
from jax.experimental import pallas as pl
from jax.experimental.pallas import tpu as pltpu

B, SQ, SKV, DM = 2, 128, 128, 512
HL, DH = 4, 64
RB = 64
NR = B * SQ // RB
HR = RB // 2
QC = 128
CR = 8
NS = RB // CR
NC = 4 * NS
BF = jnp.bfloat16
F32 = jnp.float32
MESH = pl.DeviceIdType.MESH
LOG2E = 1.4426950408889634
QS = 0.125 * LOG2E
NEG = -1e9 * LOG2E


def _make(loads, progs, pre):
    names = sorted(set(loads["E"].split() + loads["O"].split()))

    def body(x_hbm, wq_hbm, kt_hbm, vt_hbm, wo_hbm, o_ref,
             x_v, wq_v, kt_v, vt_v, wo_v, keep, sbuf, rbuf, lsem, ssem, rsem):
        me = lax.axis_index("i")
        odd = me & 1
        b = me >> 1
        kbat = (odd ^ b, b)
        peers = (me ^ 1, 3 - me)
        first = jnp.where(me == 0, 1, 0)

        def slot(role, j):
            return j // 2 if role == "E" else j % 2

        def batch(role, i):
            return i if role == "O" else (first if i == 0 else 1 - first)

        def half(j):
            return b if j in (0, 3) else 1 - b

        def pieces(role, j, q):
            if role == "E":
                return [((2 * k + s) * CR, s, q * NS + (j % 2) * (NS // 2) + k, peers[s])
                        for k in range(NS // 2) for s in range(2)]
            return [(k * CR, half(j), q * NS + k, 0 if j == 0 else 2) for k in range(NS)]

        def load(role, name):
            k, i = name[0], int(name[1])
            sem = lsem.at[names.index(name)]
            if k == "x":
                xb = x_hbm.at[batch(role, slot(role, i))]
                return pltpu.make_async_copy(xb.at[:, i % 2] if role == "E" else xb.at[half(i)], x_v.at[i], sem)
            if k == "q":
                sl = pl.ds(i * 256, 256)
                return pltpu.make_async_copy(wq_hbm.at[sl], wq_v.at[sl], sem)
            if k == "o":
                sl = pl.ds(i * QC, QC)
                return pltpu.make_async_copy(wo_hbm.at[:, sl], wo_v.at[:, sl], sem)
            src, dst = (kt_hbm, kt_v) if k == "k" else (vt_hbm, vt_v)
            return pltpu.make_async_copy(src.at[batch(role, i), pl.ds(me * HL, HL)], dst.at[i], sem)

        for role, parity in (("E", 0), ("O", 1)):
            @pl.when(odd == parity)
            def _():
                for n in loads[role].split():
                    load(role, n).start()

        bsem = pltpu.get_barrier_semaphore()
        for p in peers:
            pl.semaphore_signal(bsem, inc=1, device_id=(p,), device_id_type=MESH)

        def rdma(ph, s, c, peer):
            return pltpu.make_async_remote_copy(
                sbuf.at[ph, s, c], rbuf.at[ph, s, c], ssem, rsem.at[ph, s, c],
                device_id=(peer,), device_id_type=MESH)

        key = lax.broadcasted_iota(jnp.int32, (RB, SKV), 1)
        zpad = jnp.zeros((DH, SKV), F32)

        def cat(vs):
            return vs[0] if len(vs) == 1 else jnp.concatenate(vs, axis=0)

        def split(v, n):
            return [v[i * RB:(i + 1) * RB] for i in range(n)]

        def padded(ref, i, h, low=False):
            t = ref[i, h]
            return cat([t, zpad] if low or h % 2 == 0 else [zpad, t]).astype(BF)

        def xrows(role, js, cl):
            if role == "E":
                return cat([x_v[j, s, k * CR:(k + 1) * CR, cl]
                            for j in js for k in range(NS // 2) for s in range(2)]).astype(BF)
            return cat([x_v[j, s, :, cl] for j in js for s in range(2)]).astype(BF)

        def qsplit(q, n):
            return [[t[:, :128], t[:, 128:]] for t in split(q * QS, n)]

        def q_full(role, js, _):
            return qsplit(jnp.dot(xrows(role, js, slice(0, DM)), wq_v[...].astype(BF),
                                  preferred_element_type=F32), len(js))

        def q_lo(role, js, _):
            return split(jnp.dot(xrows(role, js, slice(0, 256)), wq_v[:256].astype(BF),
                                 preferred_element_type=F32), len(js))

        def q_hi(role, js, acc):
            return qsplit(cat(acc) + jnp.dot(xrows(role, js, slice(256, DM)), wq_v[256:].astype(BF),
                                             preferred_element_type=F32), len(js))

        def scores(role, js, qs):
            q = [cat([t[i] for t in qs]) for i in range(2)]
            ss = [split(jnp.dot(q[h // 2].astype(BF), padded(kt_v, slot(role, js[0]), h),
                                preferred_element_type=F32), len(js)) for h in range(HL)]
            return [[ss[h][i] for h in range(HL)] for i in range(len(js))]

        def sub_max(role, js, sss):
            out = []
            for j, ss in zip(js, sss):
                ds = []
                for s in ss:
                    if role == "E":
                        s = cat([s[i * CR:(i + 1) * CR] if i % 2 else
                                 jnp.where(key[:CR] < RB, s[i * CR:(i + 1) * CR], NEG) for i in range(NS)])
                    else:
                        s = jnp.where(key < RB + RB * half(j), s, NEG)
                    ds.append(s - jnp.max(s, axis=-1, keepdims=True))
                out.append(ds)
            return out

        def expo(role, js, dss):
            return [[jnp.exp2(d) for d in ds] for ds in dss]

        def weights(role, js, sss):
            return expo(role, js, sub_max(role, js, sss))

        def pv(role, js, ess, low):
            os_ = []
            for h in range(HL):
                e = cat([es[h] for es in ess])
                l = jnp.sum(e, axis=-1, keepdims=True)
                o = lax.dot_general(e.astype(BF), padded(vt_v, slot(role, js[0]), h, low),
                                    (((1,), (1,)), ((), ())), preferred_element_type=F32)
                r = pl.reciprocal(l, approx=True)
                os_.append(o * (r * (2.0 - l * r)))
            return os_

        def ctx_pair(role, js, ess):
            os_ = pv(role, js, ess, False)
            cs = [split(os_[2 * i] + os_[2 * i + 1], len(js)) for i in range(2)]
            return [[cs[0][i], cs[1][i]] for i in range(len(js))]

        def ctx_head(role, js, ess):
            hs = [split(o, len(js)) for o in pv(role, js, ess, True)]
            return [[None, None, [hs[h][i] for h in range(HL)]] for i in range(len(js))]

        def join(role, js, vs):
            return [[v[2][0] + pltpu.roll(v[2][1], DH, 1), v[2][2] + pltpu.roll(v[2][3], DH, 1), v[2]] for v in vs]

        def ctx_both(role, js, ess):
            os_ = pv(role, js, ess, True)
            cs = [split(os_[2 * i] + pltpu.roll(os_[2 * i + 1], DH, 1), len(js)) for i in range(2)]
            hs = [split(o, len(js)) for o in os_]
            return [[cs[0][i], cs[1][i], [hs[h][i] for h in range(HL)]] for i in range(len(js))]

        stage = dict(A=q_full, a=q_lo, b=q_hi, B=scores, M=sub_max, X=expo, C=weights,
                     D=ctx_pair, e=ctx_head, J=join, E=ctx_both)

        def project(val, js, cl, per_head):
            if per_head:
                zw = jnp.zeros((DH, cl.stop - cl.start), F32)
                ps = [jnp.dot(cat([val[j][2][h] for j in js]).astype(BF),
                              cat([wo_v[h * DH:(h + 1) * DH, cl], zw]).astype(BF),
                              preferred_element_type=F32) for h in range(HL)]
                return split((ps[0] + ps[1]) + (ps[2] + ps[3]), len(js))
            return split(sum(jnp.dot(cat([val[j][i] for j in js]).astype(BF),
                                     wo_v[i * 128:(i + 1) * 128, cl].astype(BF),
                                     preferred_element_type=F32) for i in range(2)), len(js))

        def sel(pair, s):
            return jnp.where(s == 0, pair[0], pair[1])

        s2 = jnp.where(odd == 1, 1 - b, 0)
        ord2, ord3 = (s2, 1 - s2), (1 - s2, s2)
        p2 = [sel(peers, 1 - s) for s in ord2]

        def phase2(cs):
            for c in cs:
                for s, peer in zip(ord2, p2):
                    rdma(0, s, c, 0).wait_recv()
                    t = keep[s, c] + rbuf[0, s, c].astype(F32)
                    keep[s, c] = t
                    sbuf[1, s, c] = t.astype(BF)
                    rdma(1, s, c, peer).start()

        def run(role):
            val, out = [None] * NR, {}
            for tok in progs[role].split():
                k = tok[0]
                if k == "w":
                    for n in tok[1:].split(","):
                        load(role, n).wait()
                elif tok == "bar":
                    pl.semaphore_wait(bsem, 2)
                elif k == "P":
                    lo, hi = tok[1:].split("-")
                    phase2(range(int(lo), int(hi)))
                elif "." not in tok:
                    js = [int(r) for r in tok[1:]]
                    for j, v in zip(js, stage[k](role, js, [val[j] for j in js])):
                        val[j] = v
                else:
                    js, qs = [[int(r) for r in t] for t in tok[1:].split(".")]
                    if k in "GHFIK":
                        cl = slice(qs[0] * QC, (qs[-1] + 1) * QC)
                        for j, g in zip(js, project(val, js, cl, k in "HI")):
                            for i, q in enumerate(qs):
                                gq = g[:, i * QC:(i + 1) * QC]
                                out[j, q] = gq.astype(BF) if k in "GH" else gq
                        if k != "K":
                            continue
                    for q in qs:
                        ps = [(j, p) for ps in zip(*[pieces(role, j, q) for j in js]) for j, p in zip(js, ps)]
                        sums = []
                        for j, (r, s, c, peer) in ps:
                            if k in "KT":
                                keep[s, c] = out[j, q][r:r + CR]
                            elif k == "S":
                                sbuf[0, s, c] = out[j, q][r:r + CR]
                                rdma(0, s, c, peer).start()
                            elif k == "R":
                                rdma(0, s, c, 0).wait_recv()
                            else:
                                assert k == "Q" and role == "E"
                                t = out[j, q][r:r + CR] + rbuf[0, s, c].astype(F32)
                                sbuf[1, s, c] = t.astype(BF)
                                rdma(1, s, c, peers[1 - s]).start()
                                sums.append((s, c, t))
                        for s, c, t in sums:
                            keep[s, c] = t

        for role, parity in (("E", 0), ("O", 1)):
            @pl.when(odd == parity)
            def _():
                run(role)

        phase2(range(pre, NC))

        def out_at(bt, s, c):
            return (bt, s, pl.ds((c % NS) * CR, CR), pl.ds((c // NS) * QC, QC))

        p3 = [sel(peers, s) for s in ord3]
        kb3 = [sel(kbat, s) for s in ord3]
        for c in range(NC):
            for s, peer, bt in zip(ord3, p3, kb3):
                rdma(1, s, c, 0).wait_recv()
                t = keep[s, c] + rbuf[1, s, c].astype(F32)
                sbuf[2, s, c] = t.astype(BF)
                rdma(2, s, c, peer).start()
                o_ref[out_at(bt, s, c)] = t

        for c in range(NC):
            if c == NC - 1:
                pltpu.make_async_copy(sbuf, sbuf, ssem).wait()
            for s in range(2):
                rdma(2, s, c, 0).wait_recv()
                o_ref[out_at(1 - kbat[s], s, c)] = rbuf[2, s, c].astype(F32)

    def kernel(x, Wq, K_ext, V_ext, Wo):
        return pl.pallas_call(
            body,
            out_shape=jax.ShapeDtypeStruct((B, 2, RB, DM), F32),
            in_specs=[pl.BlockSpec(memory_space=pl.ANY)] * 5,
            out_specs=pl.BlockSpec(memory_space=pltpu.VMEM),
            scratch_shapes=[
                pltpu.VMEM((NR, 2, HR, DM), F32),
                pltpu.VMEM((DM, HL * DH), F32),
                pltpu.VMEM((B, HL, DH, SKV), F32),
                pltpu.VMEM((B, HL, DH, SKV), F32),
                pltpu.VMEM((HL * DH, DM), F32),
                pltpu.VMEM((2, NC, CR, QC), F32),
                pltpu.VMEM((3, 2, NC, CR, QC), BF),
                pltpu.VMEM((3, 2, NC, CR, QC), BF),
                pltpu.SemaphoreType.DMA((len(names),)),
                pltpu.SemaphoreType.DMA,
                pltpu.SemaphoreType.DMA((3, 2, NC)),
            ],
            compiler_params=pltpu.CompilerParams(
                collective_id=0, disable_bounds_checks=True, disable_semaphore_checks=True),
        )(x.reshape(B, 2, 2, HR, DM), Wq, jnp.transpose(K_ext, (0, 2, 3, 1)),
          jnp.transpose(V_ext, (0, 2, 3, 1)), Wo).reshape(B, SQ, DM)

    return kernel


_KERNEL = _make(
    loads=dict(E="q0 x0 x1 q1 k0 v0 o0 x2 o1 x3 o2 k1 o3 v1",
               O="q0 x0 x1 q1 k0 v0 k1 o0 v1 o1 x2 x3 o2 o3"),
    progs=dict(E="wx0,x1,q0 a01 wq1 b01 wk0 B01 M0 wv0 X0 e0 wo0 bar H0.0 C1 E1 H1.0 J0 S0.0 S1.0 "
                 "wx2,o1 G0.1 G1.1 A2 S0.1 S1.1 wx3,o2 G0.2 G1.2 A3 S0.2 S1.2 "
                 "wk1 B2 wo3 G0.3 G1.3 C2 B3 S0.3 S1.3 "
                 "wv1 R2.0 e2 I2.0 C3 e3 I3.0 J2 Q2.0 T3.0 P4-8 "
                 "R2.1 F2.1 I3.1 J3 Q2.1 T3.1 P12-16 K23.2 P16-23 K23.3",
               O="wx0,x1,q0 a01 wq1 b01 wk0 B0 C0 wv0,k1 B1 D0 C1 wo0 bar G0.0 S0.0 wv1 E1 H1.0 S1.0 "
                 "wo1,x2 G0.1 G1.1 A2 S01.1 B2 wx3,o2 G0.2 G1.2 A3 C2 D2 S01.2 "
                 "wo3 G0.3 G1.3 B3 F2.0123 C3 D3 S01.3 T2.0123 K3.0123 P0-23"),
    pre=23)


def pallas_dist_sparse_attn_blocksparse_htp_b2_sq128_skv128_hq4_dh64_kernel(x, Wq, K_ext, V_ext, Wo):
    return _KERNEL(x, Wq, K_ext, V_ext, Wo)
```

```python
import jax
import jax.numpy as jnp
from jax import lax
from jax.experimental import pallas as pl
from jax.experimental.pallas import tpu as pltpu

B, SQ, SKV, DM = 2, 128, 128, 512
HL, DH = 4, 64
RB = 64
NR = B * SQ // RB
HR = RB // 2
QC = 128
CR = 8
NS = RB // CR
NC = 4 * NS
BF = jnp.bfloat16
F32 = jnp.float32
MESH = pl.DeviceIdType.MESH
LOG2E = 1.4426950408889634
QS = 0.125 * LOG2E
NEG = -1e9 * LOG2E


def _make(loads, progs, pre):
    names = sorted(set(loads["E"].split() + loads["O"].split()))

    def body(x_hbm, wq_hbm, kt_hbm, vt_hbm, wo_hbm, o_ref,
             x_v, wq_v, kt_v, vt_v, wo_v, keep, sbuf, rbuf, lsem, ssem, rsem, osem):
        me = lax.axis_index("i")
        odd = me & 1
        b = me >> 1
        kbat = (odd ^ b, b)
        peers = (me ^ 1, 3 - me)
        first = jnp.where(me == 0, 1, 0)

        def slot(role, j):
            return j // 2 if role == "E" else j % 2

        def batch(role, i):
            return i if role == "O" else (first if i == 0 else 1 - first)

        def half(j):
            return b if j in (0, 3) else 1 - b

        def pieces(role, j, q):
            if role == "E":
                return [((2 * k + s) * CR, s, q * NS + (j % 2) * (NS // 2) + k, peers[s])
                        for k in range(NS // 2) for s in range(2)]
            return [(k * CR, half(j), q * NS + k, 0 if j == 0 else 2) for k in range(NS)]

        def load(role, name):
            k, i = name[0], int(name[1])
            sem = lsem.at[names.index(name)]
            if k == "x":
                xb = x_hbm.at[batch(role, slot(role, i))]
                return pltpu.make_async_copy(xb.at[:, i % 2] if role == "E" else xb.at[half(i)], x_v.at[i], sem)
            if k == "q":
                sl = pl.ds(i * 256, 256)
                return pltpu.make_async_copy(wq_hbm.at[sl], wq_v.at[sl], sem)
            if k == "o":
                sl = pl.ds(i * QC, QC)
                return pltpu.make_async_copy(wo_hbm.at[:, sl], wo_v.at[:, sl], sem)
            src, dst = (kt_hbm, kt_v) if k == "k" else (vt_hbm, vt_v)
            return pltpu.make_async_copy(src.at[batch(role, i), pl.ds(me * HL, HL)], dst.at[i], sem)

        for role, parity in (("E", 0), ("O", 1)):
            @pl.when(odd == parity)
            def _():
                for n in loads[role].split():
                    load(role, n).start()

        bsem = pltpu.get_barrier_semaphore()
        for p in peers:
            pl.semaphore_signal(bsem, inc=1, device_id=(p,), device_id_type=MESH)

        def rdma(ph, s, c, peer):
            return pltpu.make_async_remote_copy(
                sbuf.at[ph, s, c], rbuf.at[ph, s, c], ssem, rsem.at[ph, s, c],
                device_id=(peer,), device_id_type=MESH)

        key = lax.broadcasted_iota(jnp.int32, (RB, SKV), 1)
        zpad = jnp.zeros((DH, SKV), F32)

        def cat(vs):
            return vs[0] if len(vs) == 1 else jnp.concatenate(vs, axis=0)

        def split(v, n):
            return [v[i * RB:(i + 1) * RB] for i in range(n)]

        def padded(ref, i, h, low=False):
            t = ref[i, h]
            return cat([t, zpad] if low or h % 2 == 0 else [zpad, t]).astype(BF)

        def xrows(role, js, cl):
            if role == "E":
                return cat([x_v[j, s, k * CR:(k + 1) * CR, cl]
                            for j in js for k in range(NS // 2) for s in range(2)]).astype(BF)
            return cat([x_v[j, s, :, cl] for j in js for s in range(2)]).astype(BF)

        def qsplit(q, n):
            return [[t[:, :128], t[:, 128:]] for t in split(q * QS, n)]

        def q_full(role, js, _):
            return qsplit(jnp.dot(xrows(role, js, slice(0, DM)), wq_v[...].astype(BF),
                                  preferred_element_type=F32), len(js))

        def q_lo(role, js, _):
            return split(jnp.dot(xrows(role, js, slice(0, 256)), wq_v[:256].astype(BF),
                                 preferred_element_type=F32), len(js))

        def q_hi(role, js, acc):
            return qsplit(cat(acc) + jnp.dot(xrows(role, js, slice(256, DM)), wq_v[256:].astype(BF),
                                             preferred_element_type=F32), len(js))

        def scores(role, js, qs):
            q = [cat([t[i] for t in qs]) for i in range(2)]
            ss = [split(jnp.dot(q[h // 2].astype(BF), padded(kt_v, slot(role, js[0]), h),
                                preferred_element_type=F32), len(js)) for h in range(HL)]
            return [[ss[h][i] for h in range(HL)] for i in range(len(js))]

        def sub_max(role, js, sss):
            out = []
            for j, ss in zip(js, sss):
                ds = []
                for s in ss:
                    if role == "E":
                        s = cat([s[i * CR:(i + 1) * CR] if i % 2 else
                                 jnp.where(key[:CR] < RB, s[i * CR:(i + 1) * CR], NEG) for i in range(NS)])
                    else:
                        s = jnp.where(key < RB + RB * half(j), s, NEG)
                    ds.append(s - jnp.max(s, axis=-1, keepdims=True))
                out.append(ds)
            return out

        def expo(role, js, dss):
            return [[jnp.exp2(d) for d in ds] for ds in dss]

        def weights(role, js, sss):
            return expo(role, js, sub_max(role, js, sss))

        def pv(role, js, ess, low):
            os_ = []
            for h in range(HL):
                e = cat([es[h] for es in ess])
                l = jnp.sum(e, axis=-1, keepdims=True)
                o = lax.dot_general(e.astype(BF), padded(vt_v, slot(role, js[0]), h, low),
                                    (((1,), (1,)), ((), ())), preferred_element_type=F32)
                r = pl.reciprocal(l, approx=True)
                os_.append(o * (r * (2.0 - l * r)))
            return os_

        def ctx_pair(role, js, ess):
            os_ = pv(role, js, ess, False)
            cs = [split(os_[2 * i] + os_[2 * i + 1], len(js)) for i in range(2)]
            return [[cs[0][i], cs[1][i]] for i in range(len(js))]

        def ctx_head(role, js, ess):
            hs = [split(o, len(js)) for o in pv(role, js, ess, True)]
            return [[None, None, [hs[h][i] for h in range(HL)]] for i in range(len(js))]

        def join(role, js, vs):
            return [[v[2][0] + pltpu.roll(v[2][1], DH, 1), v[2][2] + pltpu.roll(v[2][3], DH, 1), v[2]] for v in vs]

        def ctx_both(role, js, ess):
            os_ = pv(role, js, ess, True)
            cs = [split(os_[2 * i] + pltpu.roll(os_[2 * i + 1], DH, 1), len(js)) for i in range(2)]
            hs = [split(o, len(js)) for o in os_]
            return [[cs[0][i], cs[1][i], [hs[h][i] for h in range(HL)]] for i in range(len(js))]

        stage = dict(A=q_full, a=q_lo, b=q_hi, B=scores, M=sub_max, X=expo, C=weights,
                     D=ctx_pair, e=ctx_head, J=join, E=ctx_both)

        def project(val, js, cl, per_head):
            if per_head:
                zw = jnp.zeros((DH, cl.stop - cl.start), F32)
                ps = [jnp.dot(cat([val[j][2][h] for j in js]).astype(BF),
                              cat([wo_v[h * DH:(h + 1) * DH, cl], zw]).astype(BF),
                              preferred_element_type=F32) for h in range(HL)]
                return split((ps[0] + ps[1]) + (ps[2] + ps[3]), len(js))
            return split(sum(jnp.dot(cat([val[j][i] for j in js]).astype(BF),
                                     wo_v[i * 128:(i + 1) * 128, cl].astype(BF),
                                     preferred_element_type=F32) for i in range(2)), len(js))

        def sel(pair, s):
            return jnp.where(s == 0, pair[0], pair[1])

        s2 = jnp.where(odd == 1, 1 - b, 0)
        ord2, ord3 = (s2, 1 - s2), (1 - s2, s2)
        p2 = [sel(peers, 1 - s) for s in ord2]

        def phase2(cs):
            for c in cs:
                for s, peer in zip(ord2, p2):
                    rdma(0, s, c, 0).wait_recv()
                    t = keep[s, c] + rbuf[0, s, c].astype(F32)
                    keep[s, c] = t
                    sbuf[1, s, c] = t.astype(BF)
                    rdma(1, s, c, peer).start()

        def run(role):
            val, out = [None] * NR, {}
            for tok in progs[role].split():
                k = tok[0]
                if k == "w":
                    for n in tok[1:].split(","):
                        load(role, n).wait()
                elif tok == "bar":
                    pl.semaphore_wait(bsem, 2)
                elif k == "P":
                    lo, hi = tok[1:].split("-")
                    phase2(range(int(lo), int(hi)))
                elif "." not in tok:
                    js = [int(r) for r in tok[1:]]
                    for j, v in zip(js, stage[k](role, js, [val[j] for j in js])):
                        val[j] = v
                else:
                    js, qs = [[int(r) for r in t] for t in tok[1:].split(".")]
                    if k in "GHFIK":
                        cl = slice(qs[0] * QC, (qs[-1] + 1) * QC)
                        for j, g in zip(js, project(val, js, cl, k in "HI")):
                            for i, q in enumerate(qs):
                                gq = g[:, i * QC:(i + 1) * QC]
                                out[j, q] = gq.astype(BF) if k in "GH" else gq
                        if k != "K":
                            continue
                    for q in qs:
                        ps = [(j, p) for ps in zip(*[pieces(role, j, q) for j in js]) for j, p in zip(js, ps)]
                        sums = []
                        for j, (r, s, c, peer) in ps:
                            if k in "KT":
                                keep[s, c] = out[j, q][r:r + CR]
                            elif k == "S":
                                sbuf[0, s, c] = out[j, q][r:r + CR]
                                rdma(0, s, c, peer).start()
                            elif k == "R":
                                rdma(0, s, c, 0).wait_recv()
                            else:
                                assert k == "Q" and role == "E"
                                t = out[j, q][r:r + CR] + rbuf[0, s, c].astype(F32)
                                sbuf[1, s, c] = t.astype(BF)
                                rdma(1, s, c, peers[1 - s]).start()
                                sums.append((s, c, t))
                        for s, c, t in sums:
                            keep[s, c] = t

        for role, parity in (("E", 0), ("O", 1)):
            @pl.when(odd == parity)
            def _():
                run(role)

        phase2(range(pre, NC))

        p3 = [sel(peers, s) for s in ord3]
        kb3 = [sel(kbat, s) for s in ord3]
        for c in range(NC):
            for s, peer, bt in zip(ord3, p3, kb3):
                at = (bt, s, pl.ds((c % NS) * CR, CR), pl.ds((c // NS) * QC, QC))
                rdma(1, s, c, 0).wait_recv()
                o_ref[at] = (keep[s, c] + rbuf[1, s, c].astype(F32)).astype(BF)
                pltpu.make_async_remote_copy(o_ref.at[at], o_ref.at[at], osem.at[0, s], osem.at[1, s],
                                             device_id=(peer,), device_id_type=MESH).start()

        pltpu.make_async_copy(sbuf, sbuf, ssem).wait()
        for d in range(2):
            for s in range(2):
                rows = o_ref.at[kbat[s] ^ d, s]
                pltpu.make_async_copy(rows, rows, osem.at[d, s]).wait()

    def kernel(x, Wq, K_ext, V_ext, Wo):
        return pl.pallas_call(
            body,
            out_shape=jax.ShapeDtypeStruct((B, 2, RB, DM), BF),
            in_specs=[pl.BlockSpec(memory_space=pl.ANY)] * 5,
            out_specs=pl.BlockSpec(memory_space=pltpu.VMEM),
            scratch_shapes=[
                pltpu.VMEM((NR, 2, HR, DM), F32),
                pltpu.VMEM((DM, HL * DH), F32),
                pltpu.VMEM((B, HL, DH, SKV), F32),
                pltpu.VMEM((B, HL, DH, SKV), F32),
                pltpu.VMEM((HL * DH, DM), F32),
                pltpu.VMEM((2, NC, CR, QC), F32),
                pltpu.VMEM((2, 2, NC, CR, QC), BF),
                pltpu.VMEM((2, 2, NC, CR, QC), BF),
                pltpu.SemaphoreType.DMA((len(names),)),
                pltpu.SemaphoreType.DMA,
                pltpu.SemaphoreType.DMA((2, 2, NC)),
                pltpu.SemaphoreType.DMA((2, 2)),
            ],
            compiler_params=pltpu.CompilerParams(
                collective_id=0, disable_bounds_checks=True, disable_semaphore_checks=True),
        )(x.reshape(B, 2, 2, HR, DM), Wq, jnp.transpose(K_ext, (0, 2, 3, 1)),
          jnp.transpose(V_ext, (0, 2, 3, 1)), Wo).reshape(B, SQ, DM)

    return kernel


_KERNEL = _make(
    loads=dict(E="q0 x0 x1 q1 k0 v0 o0 x2 o1 x3 o2 k1 o3 v1",
               O="q0 x0 x1 q1 k0 v0 k1 o0 v1 o1 x2 x3 o2 o3"),
    progs=dict(E="wx0,x1,q0 a01 wq1 b01 wk0 B01 M0 wv0 X0 e0 wo0 bar H0.0 C1 E1 H1.0 J0 S0.0 S1.0 "
                 "wx2,o1 G0.1 G1.1 A2 S0.1 S1.1 wx3,o2 G0.2 G1.2 A3 S0.2 S1.2 "
                 "wk1 B2 wo3 G0.3 G1.3 C2 B3 S0.3 S1.3 "
                 "wv1 R2.0 e2 I2.0 C3 e3 I3.0 J2 Q2.0 T3.0 P4-8 "
                 "R2.1 F2.1 I3.1 J3 Q2.1 T3.1 P12-16 K23.2 P16-23 K23.3",
               O="wx0,x1,q0 a01 wq1 b01 wk0 B0 C0 wv0,k1 B1 D0 C1 wo0 bar G0.0 S0.0 wv1 E1 H1.0 S1.0 "
                 "wo1,x2 G0.1 G1.1 A2 S01.1 B2 wx3,o2 G0.2 G1.2 A3 C2 D2 S01.2 "
                 "wo3 G0.3 G1.3 B3 F2.0123 C3 D3 S01.3 T2.0123 K3.0123 P0-23"),
    pre=23)


def pallas_dist_sparse_attn_blocksparse_htp_b2_sq128_skv128_hq4_dh64_kernel(x, Wq, K_ext, V_ext, Wo):
    return _KERNEL(x, Wq, K_ext, V_ext, Wo)
```
